```python
import numpy as np

kernel_name = "dist_rope_attn_htp_bs_b2_sq512_d1024_hq8_dh128"

def setup_inputs():
    x = np.random.randn(8, 512, 1024).astype(np.float32)
    Wq = np.random.randn(1024, 4096).astype(np.float32) * 0.02
    Wk = np.random.randn(1024, 4096).astype(np.float32) * 0.02
    Wv = np.random.randn(1024, 4096).astype(np.float32) * 0.02
    Wo = np.random.randn(4096, 1024).astype(np.float32) * 0.02
    return {"x": x, "Wq": Wq, "Wk": Wk, "Wv": Wv, "Wo": Wo}

def reference(x, Wq, Wk, Wv, Wo):
    B, Sq, Hq, Dh = 8, 512, 32, 128
    inv = 1.0 / (10000.0 ** (np.arange(0, Dh, 2) / Dh))
    pos = np.arange(Sq)[:, None] * inv[None, :]
    cos = np.repeat(np.cos(pos), 2, axis=-1).astype(np.float32)
    sin = np.repeat(np.sin(pos), 2, axis=-1).astype(np.float32)
    def rot(t):
        t2 = t.reshape(B, Sq, Hq, Dh // 2, 2)
        t_r = np.stack([-t2[..., 1], t2[..., 0]], axis=-1).reshape(B, Sq, Hq, Dh)
        return t * cos[None, :, None, :] + t_r * sin[None, :, None, :]
    Q = rot((x @ Wq).reshape(B, Sq, Hq, Dh))
    K = rot((x @ Wk).reshape(B, Sq, Hq, Dh))
    V = (x @ Wv).reshape(B, Sq, Hq, Dh)
    s = np.einsum('bihd,bjhd->bhij', Q, K).astype(np.float32) * 0.08838834764831843
    s_max = s.max(axis=-1, keepdims=True)
    w = np.exp(s - s_max)
    w = w / w.sum(axis=-1, keepdims=True)
    ctx = np.einsum('bhij,bjhd->bihd', w, V).reshape(B, Sq, Hq * Dh)
    return ctx @ Wo
```

```python
import jax
import jax.numpy as jnp
from jax import lax
from jax.experimental import pallas as pl
from jax.experimental.pallas import tpu as pltpu

N_DEV = 4
B_LOC = 2
SQ = 512
D = 1024
H_LOC = 8
DH = 128
SCALE = 0.08838834764831843

_STEP_OFF = (-1, 1, -1, 1, 2, 2)
_STEP_B = (0, 0, 1, 1, 0, 1)


def pallas_dist_rope_attn_htp_bs_b2_sq512_d1024_hq8_dh128_kernel(
    x: jax.Array,
    Wq: jax.Array,
    Wk: jax.Array,
    Wv: jax.Array,
    Wo: jax.Array,
):
    bf16 = jnp.bfloat16
    f32 = jnp.float32

    def body(x_hbm, wq_hbm, wk_hbm, wv_hbm, wo_hbm, out_hbm,
             xf, wst, wbf, xall, psend, precv, obuf, own0,
             cos_ref, sin_ref, q_s, k_s, v_s, ctx_s,
             ld_sems, xs_send, xs_recv, ps_send, ps_recv, out_sems):
        me = lax.axis_index("i")

        x_ld = [pltpu.make_async_copy(x_hbm.at[b], xf.at[b], ld_sems.at[b])
                for b in range(B_LOC)]
        w_hbm = (wq_hbm, wk_hbm, wv_hbm, wo_hbm)
        w_ld = [pltpu.make_async_copy(w_hbm[j], wst.at[j], ld_sems.at[2 + j])
                for j in range(4)]
        for c in x_ld:
            c.start()
        for c in w_ld:
            c.start()

        bar = pltpu.get_barrier_semaphore()
        for d in range(1, N_DEV):
            pl.semaphore_signal(bar, inc=1, device_id=((me + d) % N_DEV,),
                                device_id_type=pl.DeviceIdType.MESH)

        lane = lax.broadcasted_iota(jnp.int32, (SQ, DH), 1)
        row = lax.broadcasted_iota(jnp.int32, (SQ, DH), 0)
        pair = (lane // 2).astype(f32)
        inv = jnp.exp(pair * (-2.0 / DH) * jnp.log(10000.0))
        ang = row.astype(f32) * inv
        even = (lane % 2) == 0
        cos_ref[...] = jnp.cos(ang)
        sn = jnp.sin(ang)
        sin_ref[...] = jnp.where(even, -sn, sn)

        pl.semaphore_wait(bar, N_DEV - 1)

        def x_copy(s):
            off, b = _STEP_OFF[s], _STEP_B[s]
            dst = (me - off) % N_DEV
            slot = B_LOC * me + b
            return pltpu.make_async_remote_copy(
                src_ref=xall.at[slot], dst_ref=xall.at[slot],
                send_sem=xs_send.at[s], recv_sem=xs_recv.at[s],
                device_id=(dst,), device_id_type=pl.DeviceIdType.MESH)

        for b in range(B_LOC):
            x_ld[b].wait()
            xall[B_LOC * me + b] = xf[b].astype(bf16)
            for s in range(6):
                if _STEP_B[s] == b:
                    x_copy(s).start()

        for j in range(4):
            w_ld[j].wait()
            wbf[j] = wst[j].astype(bf16)

        def rope(t):
            r = jnp.where(even, pltpu.roll(t, DH - 1, 1), pltpu.roll(t, 1, 1))
            return t * cos_ref[...] + r * sin_ref[...]

        def compute(slot):
            xb = xall[slot]
            q = jnp.dot(xb, wbf[0], preferred_element_type=f32)
            k = jnp.dot(xb, wbf[1], preferred_element_type=f32)
            v_s[...] = jnp.dot(xb, wbf[2], preferred_element_type=f32).astype(bf16)
            for h in range(H_LOC):
                sl = slice(h * DH, (h + 1) * DH)
                q_s[:, sl] = (rope(q[:, sl]) * SCALE).astype(bf16)
                k_s[:, sl] = rope(k[:, sl]).astype(bf16)
            for h in range(H_LOC):
                sl = slice(h * DH, (h + 1) * DH)
                s = lax.dot_general(q_s[:, sl], k_s[:, sl],
                                    (((1,), (1,)), ((), ())),
                                    preferred_element_type=f32)
                m = jnp.max(s, axis=-1, keepdims=True)
                p = jnp.exp(s - m)
                l = jnp.sum(p, axis=-1, keepdims=True)
                o = jnp.dot(p.astype(bf16), v_s[:, sl],
                            preferred_element_type=f32)
                ctx_s[:, sl] = (o / l).astype(bf16)
            return jnp.dot(ctx_s[...], wbf[3], preferred_element_type=f32)

        def p_copy(s):
            off, b = _STEP_OFF[s], _STEP_B[s]
            return pltpu.make_async_remote_copy(
                src_ref=psend.at[s], dst_ref=precv.at[s],
                send_sem=ps_send.at[s], recv_sem=ps_recv.at[s],
                device_id=((me + off) % N_DEV,),
                device_id_type=pl.DeviceIdType.MESH)

        own0[...] = compute(B_LOC * me)

        for s in range(6):
            off, b = _STEP_OFF[s], _STEP_B[s]
            x_copy(s).wait_recv()
            psend[s] = compute(B_LOC * ((me + off) % N_DEV) + b).astype(bf16)
            p_copy(s).start()

        acc = own0[...]
        for s in range(6):
            if _STEP_B[s] == 0:
                p_copy(s).wait_recv()
                acc = acc + precv[s].astype(f32)
        obuf[0] = acc
        o0 = pltpu.make_async_copy(obuf.at[0], out_hbm.at[0], out_sems.at[0])
        o0.start()

        acc = compute(B_LOC * me + 1)
        for s in range(6):
            if _STEP_B[s] == 1:
                p_copy(s).wait_recv()
                acc = acc + precv[s].astype(f32)
        obuf[1] = acc
        o1 = pltpu.make_async_copy(obuf.at[1], out_hbm.at[1], out_sems.at[1])
        o1.start()

        for s in range(6):
            x_copy(s).wait_send()
            p_copy(s).wait_send()
        o0.wait()
        o1.wait()

    any_spec = pl.BlockSpec(memory_space=pl.ANY)
    return pl.pallas_call(
        body,
        out_shape=jax.ShapeDtypeStruct((B_LOC, SQ, D), f32),
        in_specs=[any_spec] * 5,
        out_specs=any_spec,
        scratch_shapes=[
            pltpu.VMEM((B_LOC, SQ, D), f32),
            pltpu.VMEM((4, D, D), f32),
            pltpu.VMEM((4, D, D), bf16),
            pltpu.VMEM((N_DEV * B_LOC, SQ, D), bf16),
            pltpu.VMEM((6, SQ, D), bf16),
            pltpu.VMEM((6, SQ, D), bf16),
            pltpu.VMEM((B_LOC, SQ, D), f32),
            pltpu.VMEM((SQ, D), f32),
            pltpu.VMEM((SQ, DH), f32),
            pltpu.VMEM((SQ, DH), f32),
            pltpu.VMEM((SQ, D), bf16),
            pltpu.VMEM((SQ, D), bf16),
            pltpu.VMEM((SQ, D), bf16),
            pltpu.VMEM((SQ, D), bf16),
            pltpu.SemaphoreType.DMA((6,)),
            pltpu.SemaphoreType.DMA((6,)),
            pltpu.SemaphoreType.DMA((6,)),
            pltpu.SemaphoreType.DMA((6,)),
            pltpu.SemaphoreType.DMA((6,)),
            pltpu.SemaphoreType.DMA((2,)),
        ],
        compiler_params=pltpu.CompilerParams(
            collective_id=0, vmem_limit_bytes=100 * 1024 * 1024),
    )(x, Wq, Wk, Wv, Wo)
```

```python
import jax
import jax.numpy as jnp
from jax import lax
from jax.experimental import pallas as pl
from jax.experimental.pallas import tpu as pltpu

N_DEV = 4
B_LOC = 2
SQ = 512
D = 1024
H_LOC = 8
DH = 128
SCALE = 0.08838834764831843
LOG2E = 1.4426950408889634
NCS = (4, 2, 2, 1)

_STEP_OFF = (-1, 1, -1, 1, 2, 2)
_STEP_B = (0, 0, 1, 1, 0, 1)


def _off_b(r):
    off = jnp.where(r >= 4, 2, jnp.where(r % 2 == 0, -1, 1))
    b = jnp.where(r >= 4, r - 4, r // 2)
    return off, b


def pallas_dist_rope_attn_htp_bs_b2_sq512_d1024_hq8_dh128_kernel(
    x: jax.Array,
    Wq: jax.Array,
    Wk: jax.Array,
    Wv: jax.Array,
    Wo: jax.Array,
):
    bf16 = jnp.bfloat16
    f32 = jnp.float32

    def body(x_hbm, wq_hbm, wk_hbm, wv_hbm, wo_hbm, out_hbm,
             xf, wst, wbf, xall, psend, precv, obuf,
             cos_ref, sin_ref, q_s, k_s, v_s, ctx_s,
             ld_sems, xs_send, xs_recv, ps_send, ps_recv, out_sems):
        me = lax.axis_index("i")

        w_hbm = (wq_hbm, wk_hbm, wv_hbm, wo_hbm)

        def csl(j, c):
            w = D // NCS[j]
            return slice(c * w, (c + 1) * w)

        loads = [pltpu.make_async_copy(x_hbm.at[0], xf.at[0], ld_sems.at[0])]
        for j in range(4):
            if j == 3:
                loads.append(pltpu.make_async_copy(
                    x_hbm.at[1], xf.at[1], ld_sems.at[len(loads)]))
            for c in range(NCS[j]):
                loads.append(pltpu.make_async_copy(
                    w_hbm[j].at[:, csl(j, c)], wst.at[j, :, csl(j, c)],
                    ld_sems.at[len(loads)]))
        n_issued = [0]
        n_waited = [0]

        def issue(n):
            for _ in range(n):
                if n_issued[0] < len(loads):
                    loads[n_issued[0]].start()
                    n_issued[0] += 1

        def wait_next():
            loads[n_waited[0]].wait()
            n_waited[0] += 1
            issue(1)

        issue(3)

        bar = pltpu.get_barrier_semaphore()
        for d in range(1, N_DEV):
            pl.semaphore_signal(bar, inc=1, device_id=((me + d) % N_DEV,),
                                device_id_type=pl.DeviceIdType.MESH)

        lane = lax.broadcasted_iota(jnp.int32, (SQ, DH), 1)
        row = lax.broadcasted_iota(jnp.int32, (SQ, DH), 0)
        pair = (lane // 2).astype(f32)
        inv = jnp.exp(pair * (-2.0 / DH) * jnp.log(10000.0))
        ang = row.astype(f32) * inv
        cos_ref[...] = jnp.cos(ang)
        sn = jnp.sin(ang)
        sin_ref[...] = jnp.where((lane % 2) == 0, -sn, sn)

        pl.semaphore_wait(bar, N_DEV - 1)

        def x_copy(r, off, b):
            slot = B_LOC * me + b
            return pltpu.make_async_remote_copy(
                src_ref=xall.at[slot], dst_ref=xall.at[slot],
                send_sem=xs_send.at[r], recv_sem=xs_recv.at[r],
                device_id=((me - off) % N_DEV,),
                device_id_type=pl.DeviceIdType.MESH)

        def p_copy(r, off):
            return pltpu.make_async_remote_copy(
                src_ref=psend.at[r], dst_ref=precv.at[r],
                send_sem=ps_send.at[r], recv_sem=ps_recv.at[r],
                device_id=((me + off) % N_DEV,),
                device_id_type=pl.DeviceIdType.MESH)

        def send_x(b):
            xall[B_LOC * me + b] = xf[b].astype(bf16)
            for r in range(6):
                if _STEP_B[r] == b:
                    x_copy(r, _STEP_OFF[r], b).start()

        def rope(t):
            even = (lax.broadcasted_iota(jnp.int32, (SQ, DH), 1) % 2) == 0
            r = jnp.where(even, pltpu.roll(t, DH - 1, 1), pltpu.roll(t, 1, 1))
            return t * cos_ref[...] + r * sin_ref[...]

        def store_proj(j, val, c0):
            if j == 2:
                v_s[:, c0:c0 + val.shape[1]] = val.astype(bf16)
                return
            for h in range(val.shape[1] // DH):
                t = rope(val[:, h * DH:(h + 1) * DH])
                if j == 0:
                    t = t * (SCALE * LOG2E)
                    q_s[:, c0 + h * DH:c0 + (h + 1) * DH] = t.astype(bf16)
                else:
                    k_s[:, c0 + h * DH:c0 + (h + 1) * DH] = t.astype(bf16)

        def attention(heads=range(H_LOC)):
            for h in heads:
                sl = slice(h * DH, (h + 1) * DH)
                s = lax.dot_general(q_s[:, sl], k_s[:, sl],
                                    (((1,), (1,)), ((), ())),
                                    preferred_element_type=f32)
                m = jnp.max(s, axis=-1, keepdims=True)
                p = jnp.exp2(s - m)
                l = jnp.sum(p, axis=-1, keepdims=True)
                o = jnp.dot(p.astype(bf16), v_s[:, sl],
                            preferred_element_type=f32)
                ctx_s[:, sl] = (o / l).astype(bf16)

        def proj_chunk(slot, j, cols):
            t = jnp.dot(xall[slot], wbf[j, :, cols],
                        preferred_element_type=f32)
            store_proj(j, t, cols.start)

        def compute_first(slot):
            for j in range(3):
                for c in range(NCS[j]):
                    wait_next()
                    wbf[j, :, csl(j, c)] = wst[j, :, csl(j, c)].astype(bf16)
                    proj_chunk(slot, j, csl(j, c))
            wait_next()
            send_x(1)
            attention()
            for c in range(NCS[3]):
                wait_next()
                wbf[3, :, csl(3, c)] = wst[3, :, csl(3, c)].astype(bf16)
            return jnp.dot(ctx_s[...], wbf[3], preferred_element_type=f32)

        def compute(slot):
            n_pair = H_LOC // 2
            for c in range(n_pair + 1):
                if c < n_pair:
                    for j in range(3):
                        proj_chunk(slot, j, slice(c * 2 * DH, (c + 1) * 2 * DH))
                if c == n_pair:
                    ks = D - 2 * DH
                    part = jnp.dot(ctx_s[:, :ks], wbf[3, :ks, :],
                                   preferred_element_type=f32)
                if c >= 1:
                    attention(range(2 * (c - 1), 2 * c))
            return part + jnp.dot(ctx_s[:, ks:], wbf[3, ks:, :],
                                  preferred_element_type=f32)

        wait_next()
        send_x(0)
        obuf[0] = compute_first(B_LOC * me)

        def step_fn(r, carry):
            off, b = _off_b(r)
            slot = B_LOC * ((me + off) % N_DEV) + b
            pltpu.make_async_remote_copy(
                src_ref=xall.at[slot], dst_ref=xall.at[slot],
                send_sem=xs_send.at[r], recv_sem=xs_recv.at[r],
                device_id=((me + off) % N_DEV,),
                device_id_type=pl.DeviceIdType.MESH).wait_recv()
            res = compute(slot)
            psend[r] = res.astype(bf16)
            p_copy(r, off).start()
            return carry

        lax.fori_loop(0, 6, step_fn, 0)

        for r in range(6):
            if _STEP_B[r] == 0:
                p_copy(r, 0).wait_recv()
        acc = obuf[0]
        for r in range(6):
            if _STEP_B[r] == 0:
                acc = acc + precv[r].astype(f32)
        obuf[0] = acc
        o0 = pltpu.make_async_copy(obuf.at[0], out_hbm.at[0], out_sems.at[0])
        o0.start()

        acc = compute(B_LOC * me + 1)
        for r in range(6):
            if _STEP_B[r] == 1:
                p_copy(r, 0).wait_recv()
        for r in range(6):
            if _STEP_B[r] == 1:
                acc = acc + precv[r].astype(f32)
        obuf[1] = acc
        o1 = pltpu.make_async_copy(obuf.at[1], out_hbm.at[1], out_sems.at[1])
        o1.start()

        for r in range(6):
            x_copy(r, _STEP_OFF[r], _STEP_B[r]).wait_send()
            p_copy(r, _STEP_OFF[r]).wait_send()
        o0.wait()
        o1.wait()

    any_spec = pl.BlockSpec(memory_space=pl.ANY)
    return pl.pallas_call(
        body,
        out_shape=jax.ShapeDtypeStruct((B_LOC, SQ, D), f32),
        in_specs=[any_spec] * 5,
        out_specs=pl.BlockSpec(memory_space=pl.ANY),
        scratch_shapes=[
            pltpu.VMEM((B_LOC, SQ, D), f32),
            pltpu.VMEM((4, D, D), f32),
            pltpu.VMEM((4, D, D), bf16),
            pltpu.VMEM((N_DEV * B_LOC, SQ, D), bf16),
            pltpu.VMEM((6, SQ, D), bf16),
            pltpu.VMEM((6, SQ, D), bf16),
            pltpu.VMEM((B_LOC, SQ, D), f32),
            pltpu.VMEM((SQ, DH), f32),
            pltpu.VMEM((SQ, DH), f32),
            pltpu.VMEM((SQ, D), bf16),
            pltpu.VMEM((SQ, D), bf16),
            pltpu.VMEM((SQ, D), bf16),
            pltpu.VMEM((SQ, D), bf16),
            pltpu.SemaphoreType.DMA((2 + sum(NCS),)),
            pltpu.SemaphoreType.DMA((6,)),
            pltpu.SemaphoreType.DMA((6,)),
            pltpu.SemaphoreType.DMA((6,)),
            pltpu.SemaphoreType.DMA((6,)),
            pltpu.SemaphoreType.DMA((2,)),
        ],
        compiler_params=pltpu.CompilerParams(
            collective_id=0, vmem_limit_bytes=100 * 1024 * 1024),
    )(x, Wq, Wk, Wv, Wo)
```
